```python
import numpy as np

kernel_name = "dist_rope_attn_qseq_b2_sq128_d512_hq4_dh64"

def setup_inputs():
    x = np.random.randn(2, 512, 512).astype(np.float32)
    Wq = np.random.randn(512, 256).astype(np.float32) * 0.02
    Wk = np.random.randn(512, 256).astype(np.float32) * 0.02
    Wv = np.random.randn(512, 256).astype(np.float32) * 0.02
    Wo = np.random.randn(256, 512).astype(np.float32) * 0.02
    return {"x": x, "Wq": Wq, "Wk": Wk, "Wv": Wv, "Wo": Wo}

def reference(x, Wq, Wk, Wv, Wo):
    B, Sq, Hq, Dh = 2, 512, 4, 64
    inv = 1.0 / (10000.0 ** (np.arange(0, Dh, 2) / Dh))
    pos = np.arange(Sq)[:, None] * inv[None, :]
    cos = np.repeat(np.cos(pos), 2, axis=-1).astype(np.float32)
    sin = np.repeat(np.sin(pos), 2, axis=-1).astype(np.float32)
    def rot(t):
        t2 = t.reshape(B, Sq, Hq, Dh // 2, 2)
        t_r = np.stack([-t2[..., 1], t2[..., 0]], axis=-1).reshape(B, Sq, Hq, Dh)
        return t * cos[None, :, None, :] + t_r * sin[None, :, None, :]
    Q = rot((x @ Wq).reshape(B, Sq, Hq, Dh))
    K = rot((x @ Wk).reshape(B, Sq, Hq, Dh))
    V = (x @ Wv).reshape(B, Sq, Hq, Dh)
    s = np.einsum('bihd,bjhd->bhij', Q, K).astype(np.float32) * 0.125
    s_max = s.max(axis=-1, keepdims=True)
    w = np.exp(s - s_max)
    w = w / w.sum(axis=-1, keepdims=True)
    ctx = np.einsum('bhij,bjhd->bihd', w, V).reshape(B, Sq, Hq * Dh)
    return ctx @ Wo
```

```python
import jax, jax.numpy as jnp
from jax import lax
from jax.experimental import pallas as pl
from jax.experimental.pallas import tpu as pltpu

B, SQ, D, H, DH = 2, 128, 512, 4, 64
HD = H * DH
MESH = pl.DeviceIdType.MESH
NT = (((1,), (1,)), ((), ()))


def _body(x_hbm, wq_hbm, wk_hbm, wv_hbm, wo_hbm, out_ref,
          xf, wqf, wkf, wvf, wof, xg, acc_scr, st_scr, psend, pstat_send, precv, pstat_recv,
          lsem, ssem, rsem):
    my = lax.axis_index("i")
    left = (my + 3) % 4
    right = (my + 1) % 4
    b_me = my // 2
    b_left = left // 2
    b_right = right // 2

    cx = pltpu.make_async_copy(x_hbm, xf, lsem.at[0])
    cx.start()
    ck = pltpu.make_async_copy(wk_hbm, wkf, lsem.at[1])
    ck.start()
    cv = pltpu.make_async_copy(wv_hbm, wvf, lsem.at[2])
    cv.start()
    cq = pltpu.make_async_copy(wq_hbm, wqf, lsem.at[3])
    cq.start()
    co = pltpu.make_async_copy(wo_hbm, wof, lsem.at[4])
    co.start()

    bsem = pltpu.get_barrier_semaphore()
    for nb in (left, right):
        pl.semaphore_signal(bsem, inc=1, device_id=(nb,), device_id_type=MESH)
    pl.semaphore_wait(bsem, 2)

    cx.wait()
    xg[0] = xf[...].astype(jnp.bfloat16)

    def xsend(dev, dst_slot, b, si):
        return pltpu.make_async_remote_copy(
            src_ref=xg.at[0, b], dst_ref=xg.at[dst_slot, b],
            send_sem=ssem.at[si], recv_sem=rsem.at[si],
            device_id=(dev,), device_id_type=MESH)

    s_r1 = xsend(right, 1, b_right, 0)
    s_l1 = xsend(left, 2, b_left, 1)
    s_r2 = xsend(right, 1, 1 - b_right, 2)
    s_l2 = xsend(left, 2, 1 - b_left, 3)
    s_r1.start()
    s_l1.start()
    s_r2.start()
    s_l2.start()

    lane = lax.broadcasted_iota(jnp.int32, (SQ, 128), 1)
    row = lax.broadcasted_iota(jnp.int32, (SQ, 128), 0)
    lane1 = lax.broadcasted_iota(jnp.int32, (8, 128), 1)

    def inv_freq(l):
        k2 = ((l % DH) // 2 * 2).astype(jnp.float32)
        return jnp.exp(k2 * (-jnp.log(10000.0) / DH))

    inv = inv_freq(lane)
    even = (lane % 2) == 0

    def tables(owner):
        pos = (row + owner * SQ).astype(jnp.float32)
        ang = pos * inv
        c = jnp.cos(ang)
        s = jnp.sin(ang)
        return c, jnp.where(even, -s, s)

    tab = [tables(my), tables(left), tables(right)]

    def rope(t, slot):
        c, s = tab[slot]
        outs = []
        for p in range(2):
            tp = t[:, 128 * p:128 * (p + 1)]
            r_up = pltpu.roll(tp, 127, 1)
            r_dn = pltpu.roll(tp, 1, 1)
            rot = jnp.where(even, r_up, r_dn)
            outs.append(tp * c + rot * s)
        return jnp.concatenate(outs, axis=1)

    ck.wait()
    cv.wait()
    cq.wait()
    wk = wkf[...].astype(jnp.bfloat16)
    wvT = wvf[...].T.astype(jnp.bfloat16)
    wq = wqf[...].astype(jnp.bfloat16)

    rowh = lax.broadcasted_iota(jnp.int32, (128, SQ), 0) // DH

    def make_qtm(xc, slot):
        q = jnp.dot(xc, wq, preferred_element_type=jnp.float32)
        q = rope(q, slot) * 0.125
        qT = q.T
        res = []
        for h in range(H):
            p, e = h // 2, h % 2
            blk = qT[128 * p:128 * (p + 1), :]
            res.append(jnp.where(rowh == e, blk, 0.0).astype(jnp.bfloat16))
        return res

    def make_kv(xc, slot):
        k = jnp.dot(xc, wk, preferred_element_type=jnp.float32)
        k = rope(k, slot).astype(jnp.bfloat16)
        vT = lax.dot_general(wvT, xc, NT, preferred_element_type=jnp.float32).astype(jnp.bfloat16)
        return k, vT

    def block(qtm, k, vT):
        ms, ls, accs = [], [], []
        for h in range(H):
            p = h // 2
            sT = jnp.dot(k[:, 128 * p:128 * (p + 1)], qtm[h], preferred_element_type=jnp.float32)
            m = jnp.max(sT, axis=0, keepdims=True)
            pT = jnp.exp(sT - m)
            l = jnp.sum(pT, axis=0, keepdims=True)
            accT = jnp.dot(vT[DH * h:DH * (h + 1), :], pT.astype(jnp.bfloat16),
                           preferred_element_type=jnp.float32)
            ms.append(m)
            ls.append(l)
            accs.append(accT)
        return (jnp.concatenate(ms + ls, axis=0), jnp.concatenate(accs, axis=0))

    qtm_own = []
    for b in range(B):
        xc = xg[0, b]
        qtm_own.append(make_qtm(xc, 0))
        k, vT = make_kv(xc, 0)
        st, acc = block(qtm_own[b], k, vT)
        st_scr[b, 0] = st
        acc_scr[b, 0] = acc

    def recv_wait(slot, b, si):
        pltpu.make_async_remote_copy(
            src_ref=xg.at[slot, b], dst_ref=xg.at[slot, b],
            send_sem=ssem.at[si], recv_sem=rsem.at[si],
            device_id=(my,), device_id_type=MESH).wait_recv()

    recv_wait(1, b_me, 0)
    recv_wait(2, b_me, 1)
    xl = xg[1, b_me]
    xr = xg[2, b_me]
    kl, vTl = make_kv(xl, 1)
    kr, vTr = make_kv(xr, 2)
    qtm_l = make_qtm(xl, 1)
    qtm_r = make_qtm(xr, 2)
    st, acc = block(qtm_l, kr, vTr)
    psend[0] = acc.astype(jnp.bfloat16)
    pstat_send[0] = st
    st, acc = block(qtm_r, kl, vTl)
    psend[1] = acc.astype(jnp.bfloat16)
    pstat_send[1] = st

    def psends():
        res = []
        for i, dev in enumerate((left, right)):
            res.append(pltpu.make_async_remote_copy(
                src_ref=psend.at[i], dst_ref=precv.at[b_me],
                send_sem=ssem.at[4 + i], recv_sem=rsem.at[4 + i],
                device_id=(dev,), device_id_type=MESH))
            res.append(pltpu.make_async_remote_copy(
                src_ref=pstat_send.at[i], dst_ref=pstat_recv.at[b_me],
                send_sem=ssem.at[6 + i], recv_sem=rsem.at[6 + i],
                device_id=(dev,), device_id_type=MESH))
        return res
    ps = psends()
    for c_ in ps:
        c_.start()

    def sel_qtm(bdyn):
        return [jnp.where(bdyn == 0, qtm_own[0][h], qtm_own[1][h]) for h in range(H)]

    q1 = sel_qtm(b_me)
    st, acc = block(q1, kl, vTl)
    st_scr[b_me, 1] = st
    acc_scr[b_me, 1] = acc
    st, acc = block(q1, kr, vTr)
    st_scr[b_me, 2] = st
    acc_scr[b_me, 2] = acc

    b2 = 1 - b_me
    recv_wait(1, b2, 2)
    recv_wait(2, b2, 3)
    q2 = sel_qtm(b2)
    kl, vTl = make_kv(xg[1, b2], 1)
    st, acc = block(q2, kl, vTl)
    st_scr[b2, 1] = st
    acc_scr[b2, 1] = acc
    kr, vTr = make_kv(xg[2, b2], 2)
    st, acc = block(q2, kr, vTr)
    st_scr[b2, 2] = st
    acc_scr[b2, 2] = acc

    co.wait()
    wo = wof[...].astype(jnp.bfloat16)
    def precv_wait(b, si_acc, si_st):
        pltpu.make_async_remote_copy(
            src_ref=precv.at[b], dst_ref=precv.at[b],
            send_sem=ssem.at[si_acc], recv_sem=rsem.at[si_acc],
            device_id=(my,), device_id_type=MESH).wait_recv()
        pltpu.make_async_remote_copy(
            src_ref=pstat_recv.at[b], dst_ref=pstat_recv.at[b],
            send_sem=ssem.at[si_st], recv_sem=rsem.at[si_st],
            device_id=(my,), device_id_type=MESH).wait_recv()
    precv_wait(b_left, 5, 7)
    precv_wait(b_right, 4, 6)

    for b in range(B):
        sts = [st_scr[b, 0], st_scr[b, 1], st_scr[b, 2], pstat_recv[b]]
        m = sts[0][0:4]
        for s_ in sts[1:]:
            m = jnp.maximum(m, s_[0:4])
        ws = [jnp.exp(s_[0:4] - m) for s_ in sts]
        l = ws[0] * sts[0][4:8]
        for w_, s_ in zip(ws[1:], sts[1:]):
            l = l + w_ * s_[4:8]
        inv_l = 1.0 / l
        accs = [acc_scr[b, 0], acc_scr[b, 1], acc_scr[b, 2], precv[b].astype(jnp.float32)]
        ctx_rows = []
        for h in range(H):
            t = None
            for j in range(4):
                a = accs[j][DH * h:DH * (h + 1), :] * ws[j][h:h + 1, :]
                t = a if t is None else t + a
            ctx_rows.append(t * inv_l[h:h + 1, :])
        ctxT = jnp.concatenate(ctx_rows, axis=0)
        ctx = ctxT.T.astype(jnp.bfloat16)
        out_ref[b] = jnp.dot(ctx, wo, preferred_element_type=jnp.float32)

    for c_ in (s_r1, s_l1, s_r2, s_l2):
        c_.wait_send()
    for c_ in ps:
        c_.wait_send()


def pallas_dist_rope_attn_qseq_b2_sq128_d512_hq4_dh64_kernel(x, Wq, Wk, Wv, Wo):
    return pl.pallas_call(
        _body,
        out_shape=jax.ShapeDtypeStruct(x.shape, jnp.float32),
        in_specs=[pl.BlockSpec(memory_space=pl.ANY)] * 5,
        out_specs=pl.BlockSpec(memory_space=pltpu.VMEM),
        scratch_shapes=[
            pltpu.VMEM((B, SQ, D), jnp.float32),
            pltpu.VMEM((D, HD), jnp.float32),
            pltpu.VMEM((D, HD), jnp.float32),
            pltpu.VMEM((D, HD), jnp.float32),
            pltpu.VMEM((HD, D), jnp.float32),
            pltpu.VMEM((3, B, SQ, D), jnp.bfloat16),
            pltpu.VMEM((B, 3, HD, SQ), jnp.float32),
            pltpu.VMEM((B, 3, 8, SQ), jnp.float32),
            pltpu.VMEM((2, HD, SQ), jnp.bfloat16),
            pltpu.VMEM((2, 8, SQ), jnp.float32),
            pltpu.VMEM((B, HD, SQ), jnp.bfloat16),
            pltpu.VMEM((B, 8, SQ), jnp.float32),
            pltpu.SemaphoreType.DMA((5,)),
            pltpu.SemaphoreType.DMA((8,)),
            pltpu.SemaphoreType.DMA((8,)),
        ],
        compiler_params=pltpu.CompilerParams(collective_id=0, vmem_limit_bytes=64 * 1024 * 1024),
    )(x, Wq, Wk, Wv, Wo)
```

```python
import jax, jax.numpy as jnp
from jax import lax
from jax.experimental import pallas as pl
from jax.experimental.pallas import tpu as pltpu

B, SQ, D, H, DH = 2, 128, 512, 4, 64
HD = H * DH
MESH = pl.DeviceIdType.MESH
NT = (((1,), (1,)), ((), ()))
F32 = jnp.float32
BF16 = jnp.bfloat16


def _body(x_hbm, wq_hbm, wk_hbm, wv_hbm, wo_hbm, out_ref,
          xf, wqf, wkf, wvf, wof, xown, xfirst, kvown, kvrecv,
          acc_scr, st_scr, psend, pstat_send, precv, pstat_recv,
          lsem, ssem, rsem):
    my = lax.axis_index("i")
    left = (my + 3) % 4
    right = (my + 1) % 4
    b_me = my // 2
    b_left = left // 2
    b_right = right // 2

    HR = SQ // 2
    xpieces = [(b_right, 0), (b_left, 0), (b_right, HR), (b_left, HR)]
    xloads = [pltpu.make_async_copy(x_hbm.at[bb, pl.ds(r0, HR)], xf.at[bb, pl.ds(r0, HR)], lsem.at[i])
              for i, (bb, r0) in enumerate(xpieces)]
    ck = pltpu.make_async_copy(wk_hbm, wkf, lsem.at[4])
    cv = pltpu.make_async_copy(wv_hbm, wvf, lsem.at[5])
    cq = pltpu.make_async_copy(wq_hbm, wqf, lsem.at[6])
    co = pltpu.make_async_copy(wo_hbm, wof, lsem.at[7])
    for c_ in xloads + [ck, cv, cq]:
        c_.start()

    bsem = pltpu.get_barrier_semaphore()
    for nb in (left, right):
        pl.semaphore_signal(bsem, inc=1, device_id=(nb,), device_id_type=MESH)
    pl.semaphore_wait(bsem, 2)

    def rcopy(src, dst, si, dev):
        return pltpu.make_async_remote_copy(
            src_ref=src, dst_ref=dst, send_sem=ssem.at[si], recv_sem=rsem.at[si],
            device_id=(dev,), device_id_type=MESH)

    xsends = []
    for i, (bb, r0) in enumerate(xpieces):
        xloads[i].wait()
        xown[bb, pl.ds(r0, HR)] = xf[bb, pl.ds(r0, HR)].astype(BF16)
        to_right = (i % 2 == 0)
        c_ = rcopy(xown.at[bb, pl.ds(r0, HR)], xfirst.at[0 if to_right else 1, pl.ds(r0, HR)],
                   i, right if to_right else left)
        c_.start()
        xsends.append(c_)

    def rwait(buf, si):
        rcopy(buf, buf, si, my).wait_recv()

    lane = lax.broadcasted_iota(jnp.int32, (SQ, 128), 1)
    row = lax.broadcasted_iota(jnp.int32, (SQ, 128), 0)
    k2 = ((lane % DH) // 2 * 2).astype(F32)
    inv = jnp.exp(k2 * (-jnp.log(10000.0) / DH))

    sgn = jnp.where((lane % 2) == 0, -1.0, 1.0)
    base = row.astype(F32) * inv
    cb, sb = jnp.cos(base), jnp.sin(base)
    lane8 = lax.broadcasted_iota(jnp.int32, (8, 128), 1)
    inv8 = jnp.exp(((lane8 % DH) // 2 * 2).astype(F32) * (-jnp.log(10000.0) / DH))
    own8 = lax.broadcasted_iota(jnp.int32, (8, 128), 0)
    own8 = jnp.where(own8 == 0, my, jnp.where(own8 == 1, left, right)) * SQ
    off = own8.astype(F32) * inv8
    co_, so_ = jnp.cos(off), jnp.sin(off)

    def tables(i):
        c1, s1 = co_[i:i + 1, :], so_[i:i + 1, :]
        return cb * c1 - sb * s1, (sb * c1 + cb * s1) * sgn

    t_own, t_l, t_r = tables(0), tables(1), tables(2)
    tab_own = (jnp.concatenate([t_own[0], t_own[0]], axis=0), jnp.concatenate([t_own[1], t_own[1]], axis=0))
    tab_nbr = (jnp.concatenate([t_l[0], t_r[0]], axis=0), jnp.concatenate([t_l[1], t_r[1]], axis=0))
    even2 = (lax.broadcasted_iota(jnp.int32, (2 * SQ, 128), 1) % 2) == 0

    def rope(t, tab):
        c, s_ = tab
        outs = []
        for p in range(2):
            tp = t[:, 128 * p:128 * (p + 1)]
            r_up = pltpu.roll(tp, 127, 1)
            r_dn = pltpu.roll(tp, 1, 1)
            outs.append(tp * c + jnp.where(even2, r_up, r_dn) * s_)
        return jnp.concatenate(outs, axis=1)


    rowh2 = lax.broadcasted_iota(jnp.int32, (128, 2 * SQ), 0) // DH
    laneh2 = lax.broadcasted_iota(jnp.int32, (128, 2 * SQ), 1) // SQ
    diag_mask = rowh2 == laneh2

    def make_qtm(q_rope):
        qT = (q_rope * 0.125).T
        res = []
        for p in range(2):
            blk = qT[128 * p:128 * (p + 1), :]
            res.append(jnp.where(diag_mask, jnp.concatenate([blk, blk], axis=1), 0.0).astype(BF16))
        return res

    def block(qtm2, k, vT):
        ms, ls, accs = [], [], []
        for p in range(2):
            sT = jnp.dot(k[:, 128 * p:128 * (p + 1)], qtm2[p], preferred_element_type=F32)
            m = jnp.max(sT, axis=0, keepdims=True)
            pT = jnp.exp(sT - m)
            l = jnp.sum(pT, axis=0, keepdims=True)
            pb = pT.astype(BF16)
            for e in range(2):
                h = 2 * p + e
                ms.append(m[:, SQ * e:SQ * (e + 1)])
                ls.append(l[:, SQ * e:SQ * (e + 1)])
                accs.append(jnp.dot(vT[DH * h:DH * (h + 1), :], pb[:, SQ * e:SQ * (e + 1)],
                                    preferred_element_type=F32))
        return jnp.concatenate(ms + ls, axis=0), jnp.concatenate(accs, axis=0)

    def pack_kv(k, vT):
        return jnp.concatenate([k, jnp.concatenate([vT[0:128, :], vT[128:256, :]], axis=1)], axis=0)

    def unpack_kv(mv):
        return mv[0:128, :], jnp.concatenate([mv[128:256, 0:128], mv[128:256, 128:256]], axis=0)

    x2own = xown[...].reshape(2 * SQ, D)
    ck.wait()
    wk = wkf[...].astype(BF16)
    k2o = rope(jnp.dot(x2own, wk, preferred_element_type=F32), tab_own).astype(BF16)
    cv.wait()
    wvT = wvf[...].T.astype(BF16)
    vT2o = lax.dot_general(wvT, x2own, NT, preferred_element_type=F32).astype(BF16)
    kv_own = []
    for b in range(B):
        kb, vTb = k2o[SQ * b:SQ * (b + 1), :], vT2o[:, SQ * b:SQ * (b + 1)]
        kv_own.append((kb, vTb))
        kvown[b] = pack_kv(kb, vTb)
    kvsends = [rcopy(kvown.at[1 - b_right], kvrecv.at[0], 4, right),
               rcopy(kvown.at[1 - b_left], kvrecv.at[1], 5, left)]
    for c_ in kvsends:
        c_.start()
    cq.wait()
    co.start()
    wq = wqf[...].astype(BF16)
    q2o = rope(jnp.dot(x2own, wq, preferred_element_type=F32), tab_own)
    qtm_own = [make_qtm(q2o[SQ * b:SQ * (b + 1), :]) for b in range(B)]
    wqk = jnp.concatenate([wq, wk], axis=1)
    for b in range(B):
        st, acc = block(qtm_own[b], *kv_own[b])
        st_scr[b, 0] = st
        acc_scr[b, 0] = acc

    for i in range(4):
        rwait(xfirst.at[i % 2, pl.ds((i // 2) * HR, HR)], i)
    x2n = xfirst[...].reshape(2 * SQ, D)
    qk = jnp.dot(x2n, wqk, preferred_element_type=F32)
    q2, k2_ = qk[:, 0:HD], qk[:, HD:2 * HD]
    vT2 = lax.dot_general(wvT, x2n, NT, preferred_element_type=F32)
    q2 = rope(q2, tab_nbr)
    k2_ = rope(k2_, tab_nbr).astype(BF16)
    vT2 = vT2.astype(BF16)
    kl, vTl = k2_[0:SQ, :], vT2[:, 0:SQ]
    kr, vTr = k2_[SQ:2 * SQ, :], vT2[:, SQ:2 * SQ]

    def psend_pair(i, dev):
        return [rcopy(psend.at[i], precv.at[b_me], 6 + i, dev),
                rcopy(pstat_send.at[i], pstat_recv.at[b_me], 8 + i, dev)]

    st, acc = block(make_qtm(q2[0:SQ, :]), kr, vTr)
    psend[0] = acc.astype(BF16)
    pstat_send[0] = st
    psends = psend_pair(0, left)
    for c_ in psends:
        c_.start()
    st, acc = block(make_qtm(q2[SQ:2 * SQ, :]), kl, vTl)
    psend[1] = acc.astype(BF16)
    pstat_send[1] = st
    ps2 = psend_pair(1, right)
    for c_ in ps2:
        c_.start()
    psends = psends + ps2

    def sel_qtm(bdyn):
        return [jnp.where(bdyn == 0, qtm_own[0][p], qtm_own[1][p]) for p in range(2)]

    st, acc = block(sel_qtm(b_me), k2_, vT2)
    st_scr[b_me, 1] = st
    acc_scr[b_me, 1] = acc

    b2 = 1 - b_me
    rwait(kvrecv.at[0], 4)
    rwait(kvrecv.at[1], 5)
    (ka, vTa), (kb, vTb) = unpack_kv(kvrecv[0]), unpack_kv(kvrecv[1])
    st, acc = block(sel_qtm(b2), jnp.concatenate([ka, kb], axis=0),
                    jnp.concatenate([vTa, vTb], axis=1))
    st_scr[b2, 1] = st
    acc_scr[b2, 1] = acc

    co.wait()
    wo = wof[...].astype(BF16)
    rwait(precv.at[b_left], 7)
    rwait(pstat_recv.at[b_left], 9)
    rwait(precv.at[b_right], 6)
    rwait(pstat_recv.at[b_right], 8)

    for b in range(B):
        sts = [st_scr[b, 0], st_scr[b, 1], pstat_recv[b]]
        m = sts[0][0:4]
        for s_ in sts[1:]:
            m = jnp.maximum(m, s_[0:4])
        ws = [jnp.exp(s_[0:4] - m) for s_ in sts]
        l = ws[0] * sts[0][4:8]
        for w_, s_ in zip(ws[1:], sts[1:]):
            l = l + w_ * s_[4:8]
        inv_l = 1.0 / l
        accs = [acc_scr[b, 0], acc_scr[b, 1], precv[b].astype(F32)]
        ctx_rows = []
        for h in range(H):
            t = None
            for j in range(3):
                a_ = accs[j][DH * h:DH * (h + 1), :] * ws[j][h:h + 1, :]
                t = a_ if t is None else t + a_
            ctx_rows.append(t * inv_l[h:h + 1, :])
        ctxT = jnp.concatenate(ctx_rows, axis=0)
        out_ref[b] = jnp.dot(ctxT.T.astype(BF16), wo, preferred_element_type=F32)

    for c_ in xsends + kvsends + psends:
        c_.wait_send()


def pallas_dist_rope_attn_qseq_b2_sq128_d512_hq4_dh64_kernel(x, Wq, Wk, Wv, Wo):
    return pl.pallas_call(
        _body,
        out_shape=jax.ShapeDtypeStruct(x.shape, jnp.float32),
        in_specs=[pl.BlockSpec(memory_space=pl.ANY)] * 5,
        out_specs=pl.BlockSpec(memory_space=pltpu.VMEM),
        scratch_shapes=[
            pltpu.VMEM((B, SQ, D), jnp.float32),
            pltpu.VMEM((D, HD), jnp.float32),
            pltpu.VMEM((D, HD), jnp.float32),
            pltpu.VMEM((D, HD), jnp.float32),
            pltpu.VMEM((HD, D), jnp.float32),
            pltpu.VMEM((B, SQ, D), jnp.bfloat16),
            pltpu.VMEM((2, SQ, D), jnp.bfloat16),
            pltpu.VMEM((B, HD, HD), jnp.bfloat16),
            pltpu.VMEM((2, HD, HD), jnp.bfloat16),
            pltpu.VMEM((B, 2, HD, SQ), jnp.float32),
            pltpu.VMEM((B, 2, 8, SQ), jnp.float32),
            pltpu.VMEM((2, HD, SQ), jnp.bfloat16),
            pltpu.VMEM((2, 8, SQ), jnp.float32),
            pltpu.VMEM((B, HD, SQ), jnp.bfloat16),
            pltpu.VMEM((B, 8, SQ), jnp.float32),
            pltpu.SemaphoreType.DMA((8,)),
            pltpu.SemaphoreType.DMA((10,)),
            pltpu.SemaphoreType.DMA((10,)),
        ],
        compiler_params=pltpu.CompilerParams(collective_id=0, vmem_limit_bytes=64 * 1024 * 1024, disable_semaphore_checks=True),
    )(x, Wq, Wk, Wv, Wo)
```

```python
import jax, jax.numpy as jnp
from jax import lax
from jax.experimental import pallas as pl
from jax.experimental.pallas import tpu as pltpu

B, SQ, D, H, DH = 2, 128, 512, 4, 64
HD = H * DH
MESH = pl.DeviceIdType.MESH
NT = (((1,), (1,)), ((), ()))
F32 = jnp.float32
BF16 = jnp.bfloat16


def _body(x_hbm, wq_hbm, wk_hbm, wv_hbm, wo_hbm, out_ref,
          xf, wqf, wkf, wvf, wof, xown, xfirst, kvown, kvrecv,
          acc_scr, st_scr, psend, pstat_send, precv, pstat_recv, e_qk, e_vT,
          lsem, ssem, rsem):
    my = lax.axis_index("i")
    left = (my + 3) % 4
    right = (my + 1) % 4
    b_me = my // 2
    b_left = left // 2
    b_right = right // 2

    HC = D // 2
    xpieces = [(b_right, 0), (b_left, 0), (b_right, HC), (b_left, HC)]
    xloads = [pltpu.make_async_copy(x_hbm.at[bb, :, pl.ds(c0, HC)], xf.at[bb, :, pl.ds(c0, HC)], lsem.at[i])
              for i, (bb, c0) in enumerate(xpieces)]
    ck = pltpu.make_async_copy(wk_hbm, wkf, lsem.at[4])
    cv = pltpu.make_async_copy(wv_hbm, wvf, lsem.at[5])
    cq = pltpu.make_async_copy(wq_hbm, wqf, lsem.at[6])
    co = pltpu.make_async_copy(wo_hbm, wof, lsem.at[7])
    for c_ in xloads + [ck, cv, cq]:
        c_.start()

    bsem = pltpu.get_barrier_semaphore()
    for nb in (left, right):
        pl.semaphore_signal(bsem, inc=1, device_id=(nb,), device_id_type=MESH)
    pl.semaphore_wait(bsem, 2)

    def rcopy(src, dst, si, dev):
        return pltpu.make_async_remote_copy(
            src_ref=src, dst_ref=dst, send_sem=ssem.at[si], recv_sem=rsem.at[si],
            device_id=(dev,), device_id_type=MESH)

    xsends = []
    for i, (bb, c0) in enumerate(xpieces):
        xloads[i].wait()
        xown[bb, :, pl.ds(c0, HC)] = xf[bb, :, pl.ds(c0, HC)].astype(BF16)
        to_right = (i % 2 == 0)
        c_ = rcopy(xown.at[bb, :, pl.ds(c0, HC)], xfirst.at[0 if to_right else 1, :, pl.ds(c0, HC)],
                   i, right if to_right else left)
        c_.start()
        xsends.append(c_)

    def rwait(buf, si):
        rcopy(buf, buf, si, my).wait_recv()

    lane = lax.broadcasted_iota(jnp.int32, (SQ, 128), 1)
    row = lax.broadcasted_iota(jnp.int32, (SQ, 128), 0)
    k2 = ((lane % DH) // 2 * 2).astype(F32)
    inv = jnp.exp(k2 * (-jnp.log(10000.0) / DH))

    sgn = jnp.where((lane % 2) == 0, -1.0, 1.0)
    base = row.astype(F32) * inv
    cb, sb = jnp.cos(base), jnp.sin(base)
    lane8 = lax.broadcasted_iota(jnp.int32, (8, 128), 1)
    inv8 = jnp.exp(((lane8 % DH) // 2 * 2).astype(F32) * (-jnp.log(10000.0) / DH))
    own8 = lax.broadcasted_iota(jnp.int32, (8, 128), 0)
    own8 = jnp.where(own8 == 0, my, jnp.where(own8 == 1, left, right)) * SQ
    off = own8.astype(F32) * inv8
    co_, so_ = jnp.cos(off), jnp.sin(off)

    def tables(i):
        c1, s1 = co_[i:i + 1, :], so_[i:i + 1, :]
        return cb * c1 - sb * s1, (sb * c1 + cb * s1) * sgn

    t_own, t_l, t_r = tables(0), tables(1), tables(2)
    tab_own = (jnp.concatenate([t_own[0], t_own[0]], axis=0), jnp.concatenate([t_own[1], t_own[1]], axis=0))
    tab_nbr = (jnp.concatenate([t_l[0], t_r[0]], axis=0), jnp.concatenate([t_l[1], t_r[1]], axis=0))
    even2 = (lax.broadcasted_iota(jnp.int32, (2 * SQ, 128), 1) % 2) == 0

    def rope(t, tab):
        c, s_ = tab
        outs = []
        for p in range(2):
            tp = t[:, 128 * p:128 * (p + 1)]
            r_up = pltpu.roll(tp, 127, 1)
            r_dn = pltpu.roll(tp, 1, 1)
            outs.append(tp * c + jnp.where(even2, r_up, r_dn) * s_)
        return jnp.concatenate(outs, axis=1)


    rowh2 = lax.broadcasted_iota(jnp.int32, (128, 2 * SQ), 0) // DH
    laneh2 = lax.broadcasted_iota(jnp.int32, (128, 2 * SQ), 1) // SQ
    diag_mask = rowh2 == laneh2

    def make_qtm(q_rope):
        qT = (q_rope * 0.125).T
        res = []
        for p in range(2):
            blk = qT[128 * p:128 * (p + 1), :]
            res.append(jnp.where(diag_mask, jnp.concatenate([blk, blk], axis=1), 0.0).astype(BF16))
        return res

    def block(qtm2, k, vT):
        ms, ls, accs = [], [], []
        for p in range(2):
            sT = jnp.dot(k[:, 128 * p:128 * (p + 1)], qtm2[p], preferred_element_type=F32)
            m = jnp.max(sT, axis=0, keepdims=True)
            pT = jnp.exp(sT - m)
            l = jnp.sum(pT, axis=0, keepdims=True)
            pb = pT.astype(BF16)
            for e in range(2):
                h = 2 * p + e
                ms.append(m[:, SQ * e:SQ * (e + 1)])
                ls.append(l[:, SQ * e:SQ * (e + 1)])
                accs.append(jnp.dot(vT[DH * h:DH * (h + 1), :], pb[:, SQ * e:SQ * (e + 1)],
                                    preferred_element_type=F32))
        return jnp.concatenate(ms + ls, axis=0), jnp.concatenate(accs, axis=0)

    def pack_kv(k, vT):
        return jnp.concatenate([k, jnp.concatenate([vT[0:128, :], vT[128:256, :]], axis=1)], axis=0)

    def unpack_kv(mv):
        return mv[0:128, :], jnp.concatenate([mv[128:256, 0:128], mv[128:256, 128:256]], axis=0)

    x2own = xown[...].reshape(2 * SQ, D)
    ck.wait()
    wk = wkf[...].astype(BF16)
    k2o = rope(jnp.dot(x2own, wk, preferred_element_type=F32), tab_own).astype(BF16)
    cv.wait()
    wvT = wvf[...].T.astype(BF16)
    vT2o = lax.dot_general(wvT, x2own, NT, preferred_element_type=F32).astype(BF16)
    kv_own = []
    for b in range(B):
        kb, vTb = k2o[SQ * b:SQ * (b + 1), :], vT2o[:, SQ * b:SQ * (b + 1)]
        kv_own.append((kb, vTb))
        kvown[b] = pack_kv(kb, vTb)
    kvsends = [rcopy(kvown.at[1 - b_right], kvrecv.at[0], 4, right),
               rcopy(kvown.at[1 - b_left], kvrecv.at[1], 5, left)]
    for c_ in kvsends:
        c_.start()
    cq.wait()
    co.start()
    wq = wqf[...].astype(BF16)
    q2o = rope(jnp.dot(x2own, wq, preferred_element_type=F32), tab_own)
    qtm_own = [make_qtm(q2o[SQ * b:SQ * (b + 1), :]) for b in range(B)]
    wqk = jnp.concatenate([wq, wk], axis=1)
    def nbr_cols(c0):
        return xfirst[:, :, c0:c0 + HC].reshape(2 * SQ, HC)

    for i in range(2):
        rwait(xfirst.at[i, :, pl.ds(0, HC)], i)
    xa = nbr_cols(0)
    e_qk[...] = jnp.dot(xa, wqk[0:HC, :], preferred_element_type=F32)
    e_vT[...] = lax.dot_general(wvT[:, 0:HC], xa, NT, preferred_element_type=F32)
    for i in range(2):
        rwait(xfirst.at[i, :, pl.ds(HC, HC)], 2 + i)
    xb_ = nbr_cols(HC)
    qk = e_qk[...] + jnp.dot(xb_, wqk[HC:D, :], preferred_element_type=F32)
    vT2 = e_vT[...] + lax.dot_general(wvT[:, HC:D], xb_, NT, preferred_element_type=F32)
    q2, k2_ = qk[:, 0:HD], qk[:, HD:2 * HD]
    q2 = rope(q2, tab_nbr)
    k2_ = rope(k2_, tab_nbr).astype(BF16)
    vT2 = vT2.astype(BF16)
    kl, vTl = k2_[0:SQ, :], vT2[:, 0:SQ]
    kr, vTr = k2_[SQ:2 * SQ, :], vT2[:, SQ:2 * SQ]

    def psend_pair(i, dev):
        return [rcopy(psend.at[i], precv.at[b_me], 6 + i, dev),
                rcopy(pstat_send.at[i], pstat_recv.at[b_me], 8 + i, dev)]

    st, acc = block(make_qtm(q2[0:SQ, :]), kr, vTr)
    psend[0] = acc.astype(BF16)
    pstat_send[0] = st
    psends = psend_pair(0, left)
    for c_ in psends:
        c_.start()
    st, acc = block(make_qtm(q2[SQ:2 * SQ, :]), kl, vTl)
    psend[1] = acc.astype(BF16)
    pstat_send[1] = st
    ps2 = psend_pair(1, right)
    for c_ in ps2:
        c_.start()
    psends = psends + ps2

    def sel_qtm(bdyn):
        return [jnp.where(bdyn == 0, qtm_own[0][p], qtm_own[1][p]) for p in range(2)]

    for b in range(B):
        st, acc = block(qtm_own[b], *kv_own[b])
        st_scr[b, 0] = st
        acc_scr[b, 0] = acc

    st, acc = block(sel_qtm(b_me), k2_, vT2)
    st_scr[b_me, 1] = st
    acc_scr[b_me, 1] = acc

    b2 = 1 - b_me
    rwait(kvrecv.at[0], 4)
    rwait(kvrecv.at[1], 5)
    (ka, vTa), (kb, vTb) = unpack_kv(kvrecv[0]), unpack_kv(kvrecv[1])
    st, acc = block(sel_qtm(b2), jnp.concatenate([ka, kb], axis=0),
                    jnp.concatenate([vTa, vTb], axis=1))
    st_scr[b2, 1] = st
    acc_scr[b2, 1] = acc

    co.wait()
    wo = wof[...].astype(BF16)
    rwait(precv.at[b_left], 7)
    rwait(pstat_recv.at[b_left], 9)
    rwait(precv.at[b_right], 6)
    rwait(pstat_recv.at[b_right], 8)

    for b in range(B):
        sts = [st_scr[b, 0], st_scr[b, 1], pstat_recv[b]]
        m = sts[0][0:4]
        for s_ in sts[1:]:
            m = jnp.maximum(m, s_[0:4])
        ws = [jnp.exp(s_[0:4] - m) for s_ in sts]
        l = ws[0] * sts[0][4:8]
        for w_, s_ in zip(ws[1:], sts[1:]):
            l = l + w_ * s_[4:8]
        inv_l = 1.0 / l
        accs = [acc_scr[b, 0], acc_scr[b, 1], precv[b].astype(F32)]
        ctx_rows = []
        for h in range(H):
            t = None
            for j in range(3):
                a_ = accs[j][DH * h:DH * (h + 1), :] * ws[j][h:h + 1, :]
                t = a_ if t is None else t + a_
            ctx_rows.append(t * inv_l[h:h + 1, :])
        ctxT = jnp.concatenate(ctx_rows, axis=0)
        out_ref[b] = jnp.dot(ctxT.T.astype(BF16), wo, preferred_element_type=F32)

    for c_ in xsends + kvsends + psends:
        c_.wait_send()


def pallas_dist_rope_attn_qseq_b2_sq128_d512_hq4_dh64_kernel(x, Wq, Wk, Wv, Wo):
    return pl.pallas_call(
        _body,
        out_shape=jax.ShapeDtypeStruct(x.shape, jnp.float32),
        in_specs=[pl.BlockSpec(memory_space=pl.ANY)] * 5,
        out_specs=pl.BlockSpec(memory_space=pltpu.VMEM),
        scratch_shapes=[
            pltpu.VMEM((B, SQ, D), jnp.float32),
            pltpu.VMEM((D, HD), jnp.float32),
            pltpu.VMEM((D, HD), jnp.float32),
            pltpu.VMEM((D, HD), jnp.float32),
            pltpu.VMEM((HD, D), jnp.float32),
            pltpu.VMEM((B, SQ, D), jnp.bfloat16),
            pltpu.VMEM((2, SQ, D), jnp.bfloat16),
            pltpu.VMEM((B, HD, HD), jnp.bfloat16),
            pltpu.VMEM((2, HD, HD), jnp.bfloat16),
            pltpu.VMEM((B, 2, HD, SQ), jnp.float32),
            pltpu.VMEM((B, 2, 8, SQ), jnp.float32),
            pltpu.VMEM((2, HD, SQ), jnp.bfloat16),
            pltpu.VMEM((2, 8, SQ), jnp.float32),
            pltpu.VMEM((B, HD, SQ), jnp.bfloat16),
            pltpu.VMEM((B, 8, SQ), jnp.float32),
            pltpu.VMEM((2 * SQ, 2 * HD), jnp.float32),
            pltpu.VMEM((HD, 2 * SQ), jnp.float32),
            pltpu.SemaphoreType.DMA((8,)),
            pltpu.SemaphoreType.DMA((10,)),
            pltpu.SemaphoreType.DMA((10,)),
        ],
        compiler_params=pltpu.CompilerParams(collective_id=0, vmem_limit_bytes=64 * 1024 * 1024, disable_semaphore_checks=True),
    )(x, Wq, Wk, Wv, Wo)
```
